```python
import numpy as np

kernel_name = "dist_moe_top2_ep_n1024_d512_e4_h1024"

def setup_inputs():
    x = np.random.randn(1024, 512).astype(np.float32)
    router_W = np.random.randn(512, 16).astype(np.float32) * 0.1
    scores64 = x.astype(np.float64) @ router_W.astype(np.float64)
    route_idx = np.argsort(-scores64, axis=-1)[:, :2].astype(np.int32)
    expert_W = np.random.randn(16, 512, 1024).astype(np.float32) * 0.02
    return {"x": x, "router_W": router_W, "route_idx": route_idx, "expert_W": expert_W}

def reference(x, router_W, route_idx, expert_W):
    scores = x @ router_W
    s_max = scores.max(axis=-1, keepdims=True)
    probs = np.exp(scores - s_max)
    probs = probs / probs.sum(axis=-1, keepdims=True)
    out = np.zeros((1024, 1024), dtype=np.float32)
    for i in range(1024):
        e0, e1 = int(route_idx[i, 0]), int(route_idx[i, 1])
        g0, g1 = probs[i, e0], probs[i, e1]
        gs = g0 + g1
        out[i] = (g0 / gs) * (x[i] @ expert_W[e0]) + (g1 / gs) * (x[i] @ expert_W[e1])
    return out
```

```python
import jax
import jax.numpy as jnp
from jax import lax
from jax.experimental import pallas as pl
from jax.experimental.pallas import tpu as pltpu

N = 1024
D = 512
H = 1024
E = 16
EL = 4
ND = 4
NB = N // 128

TM = 160
NT = -(-N // TM)
CAPE = NT * TM
SUM0 = E * CAPE
ZROW = SUM0 + 8 * N
DUMMY = ZROW + 1
ROWS = ZROW + 2

XCH = 4
WCH = 4
WC = H // WCH

F32 = jnp.float32
BF16 = jnp.bfloat16
I32 = jnp.int32
MESH = pl.DeviceIdType.MESH

SEM_M1 = 0
SEM_FW = 10
SEM_NS = 20
NSEM = SEM_NS + 2 * NB


def _kernel(x_hbm, rwt_hbm, rit_hbm, w_hbm, out_hbm,
            x32, xbf, w32, rwt, rit, ybuf, stage, outv, metav, tabv,
            tab, sa_s, sb_s, sd_s, na_s, nb_s, nd_s, fa_s, fb_s,
            lsem, msem, osem, ssem, rsem, xsem):
    my = lax.axis_index("i")
    left = (my + 3) % ND
    right = (my + 1) % ND
    diag = (my + 2) % ND
    nbr = (left, right)

    ri_cp = pltpu.make_async_copy(rit_hbm, rit, lsem.at[0])
    rw_cp = pltpu.make_async_copy(rwt_hbm, rwt, lsem.at[1])
    ri_cp.start()
    rw_cp.start()
    xr = N // XCH
    x_cp = [pltpu.make_async_copy(x_hbm.at[pl.ds(q * xr, xr)], x32.at[pl.ds(q * xr, xr)],
                                  lsem.at[2 + q]) for q in range(XCH)]
    for cp in x_cp:
        cp.start()
    w_cp = [[pltpu.make_async_copy(w_hbm.at[s, :, pl.ds(c * WC, WC)],
                                   w32.at[s, :, pl.ds(c * WC, WC)],
                                   lsem.at[2 + XCH + s * WCH + c])
             for c in range(WCH)] for s in range(EL)]
    for s in range(EL):
        for c in range(WCH):
            w_cp[s][c].start()

    barrier = pltpu.get_barrier_semaphore()
    for n in nbr:
        pl.semaphore_signal(barrier, inc=1, device_id=(n,), device_id_type=MESH)

    ybuf[ZROW] = jnp.zeros((8, 128), BF16)

    ri_cp.wait()
    e0 = rit[0:1, :]
    e1 = rit[1:2, :]
    c0 = e0 >> 2
    c1 = e1 >> 2
    dup = e0 == e1
    d01 = (c0 - c1) & 3
    d10 = (c1 - c0) & 3
    key0 = d01 * 16 + e0
    key1 = jnp.where(dup, -1, d10 * 16 + e1)
    skey = jnp.where(d01 == 0, c0,
                     jnp.where(d10 == 1, 4 + c0, jnp.where(d10 == 3, 4 + c1, -1)))

    v64 = lax.broadcasted_iota(I32, (64, N), 0)
    v16 = lax.broadcasted_iota(I32, (16, N), 0)
    m0 = v64 == key0
    m1 = v64 == key1
    ms = v16 == skey
    oh = jnp.concatenate([jnp.where(m0 | m1, 1.0, 0.0), jnp.where(ms, 1.0, 0.0)],
                         axis=0).astype(BF16)

    tok = lax.broadcasted_iota(I32, (16, N), 1)
    bsel = jnp.where(tok < v16 * 128, 1.0, 0.0).astype(BF16)
    oh128 = jnp.concatenate([oh, jnp.zeros((48, N), BF16)], axis=0)
    tabf = lax.dot_general(bsel, oh128, (((1,), (1,)), ((), ())),
                           preferred_element_type=F32)
    tabv[...] = tabf.astype(I32)
    tab_cp = pltpu.make_async_copy(tabv, tab, msem.at[0])
    tab_cp.start()

    r_i = lax.broadcasted_iota(I32, (128, 256), 0)
    c_i = lax.broadcasted_iota(I32, (128, 256), 1)
    uo = jnp.where((r_i < c_i), 1.0, 0.0).astype(BF16)
    stacked = jnp.concatenate([oh[:, b * 128:(b + 1) * 128] for b in range(NB)], axis=0)
    pre = jnp.dot(stacked, uo, preferred_element_type=F32)
    carry = jnp.zeros((80, 128), F32)
    ranks = []
    for b in range(NB):
        blk = pre[b * 80:(b + 1) * 80]
        ranks.append(blk[:, :128] + carry)
        carry = carry + blk[:, 128:]
    t0 = carry[0:16]
    t1 = t0 + carry[16:32]
    t2 = t1 + carry[32:48]
    off = jnp.concatenate([jnp.zeros((16, 128), F32), t0, t1, t2], axis=0)
    lfull = jnp.concatenate([r[:64] + off for r in ranks], axis=1)
    sfull = jnp.concatenate([r[64:] for r in ranks], axis=1)
    lp0 = jnp.sum(jnp.where(m0, lfull, 0.0), axis=0, keepdims=True).astype(I32)
    lp1 = jnp.sum(jnp.where(m1, lfull, 0.0), axis=0, keepdims=True).astype(I32)
    srk = jnp.sum(jnp.where(ms, sfull, 0.0), axis=0, keepdims=True).astype(I32)
    pos0 = e0 * CAPE + lp0
    pos1 = jnp.where(dup, ZROW, e1 * CAPE + lp1)
    spos = SUM0 + skey * N + srk
    is_d = skey < 0
    mine_s = skey == my
    mine_n = (skey == 4 + my) | (skey == 4 + left)
    arrs = [
        jnp.where(mine_s, pos0, ZROW), jnp.where(mine_s, pos1, ZROW),
        jnp.where(mine_s, spos, DUMMY),
        jnp.where(mine_n, pos0, ZROW), jnp.where(mine_n, pos1, ZROW),
        jnp.where(mine_n, spos, DUMMY),
        jnp.where(is_d, pos0, spos), jnp.where(is_d, pos1, ZROW),
    ]
    smems = [sa_s, sb_s, sd_s, na_s, nb_s, nd_s, fa_s, fb_s]
    meta_cp = []
    for k, a in enumerate(arrs):
        for b in range(NB):
            metav[k, b:b + 1, :] = a[:, b * 128:(b + 1) * 128]
        cp = pltpu.make_async_copy(metav.at[k], smems[k], msem.at[1 + k])
        cp.start()
        meta_cp.append(cp)

    rw_cp.wait()
    rwb = rwt[...].astype(BF16)
    sc = []
    for q in range(XCH):
        x_cp[q].wait()
        xq = x32[pl.ds(q * xr, xr), :].astype(BF16)
        xbf[pl.ds(q * xr, xr), :] = xq
        sc.append(lax.dot_general(rwb, xq, (((1,), (1,)), ((), ())),
                                  preferred_element_type=F32))
    scores = jnp.concatenate(sc, axis=1)
    smax = jnp.max(scores, axis=0, keepdims=True)
    p = jnp.exp(scores - smax)
    probs = p / jnp.sum(p, axis=0, keepdims=True)
    g0 = jnp.sum(jnp.where(v16 == e0, probs, 0.0), axis=0, keepdims=True)
    g1 = jnp.sum(jnp.where(v16 == e1, probs, 0.0), axis=0, keepdims=True)
    gs = g0 + g1
    w0 = g0 / gs
    w1 = g1 / gs
    w0 = jnp.where(dup, w0 + w1, w0)

    def seg(e):
        o1 = tab[8, e]
        o2 = o1 + tab[8, 16 + e]
        o3 = o2 + tab[8, 32 + e]
        o4 = o3 + tab[8, 48 + e]
        return o1, o2, o3, o4

    def ranges(chip, s):
        if s < EL:
            e = chip * EL + s
            o1, o2, o3, o4 = seg(e)
            base = e * CAPE
        else:
            o1 = o2 = 0
            o3 = o4 = tab[8, 64 + chip]
            base = SUM0 + chip * N
        mid = o2 + ((o3 - o2) >> 1)
        return base + o1, base + o2, base + mid, base + o3, base + o4

    def rcopy(lo, hi, sem_idx, dev):
        rows = ybuf.at[pl.ds(lo, hi - lo)]
        return pltpu.make_async_remote_copy(
            src_ref=rows, dst_ref=rows, send_sem=ssem.at[sem_idx],
            recv_sem=rsem.at[sem_idx], device_id=(dev,), device_id_type=MESH)

    sent = []

    def send(lo, hi, sem_idx, d):
        @pl.when(hi > lo)
        def _():
            rcopy(lo, hi, sem_idx + d, nbr[d]).start()
        sent.append((lo, hi, sem_idx + d))

    def recv(lo, hi, sem_idx, d):
        @pl.when(hi > lo)
        def _():
            rcopy(lo, hi, sem_idx + d, my).wait_recv()

    def send_own(s):
        a, b, _, c, dd = ranges(my, s)
        send(a, c, SEM_M1 + 2 * s, 0)
        send(b, dd, SEM_M1 + 2 * s, 1)

    def recv_and_forward(s):
        a, b, m, c, _ = ranges(right, s)
        recv(a, c, SEM_M1 + 2 * s, 0)
        send(b, m, SEM_FW + 2 * s, 0)
        _, b, m, c, dd = ranges(left, s)
        recv(b, dd, SEM_M1 + 2 * s, 1)
        send(m, c, SEM_FW + 2 * s, 1)

    def recv_forwarded(s):
        _, b, m, c, _ = ranges(diag, s)
        recv(b, m, SEM_FW + 2 * s, 0)
        recv(m, c, SEM_FW + 2 * s, 1)

    jrow = lax.broadcasted_iota(I32, (TM, N), 0)

    def gather(lp, gt, i):
        pm = jnp.where(jrow == lp - i * TM, gt, 0.0).astype(BF16)
        return jnp.dot(pm, xbf[...], preferred_element_type=F32).astype(BF16)

    def expert_tile(xg, s, i, wait):
        for c in range(WCH):
            if wait:
                w_cp[s][c].wait()
            wc = w32[s, :, pl.ds(c * WC, WC)].astype(BF16)
            y = jnp.dot(xg, wc, preferred_element_type=F32)
            for k in range(WC // 128):
                stage[pl.ds(c * (WC // 128) + k, TM, stride=8), :] = y[:, k * 128:(k + 1) * 128]
        base = (my * EL + s) * CAPE + i * TM
        ybuf[pl.ds(base, TM)] = stage[...].reshape(TM, 8, 128).astype(BF16)

    for s in range(EL):
        e = my * EL + s
        hit0 = e0 == e
        lp = jnp.where(hit0, lp0, jnp.where((e1 == e) & jnp.logical_not(dup), lp1, -1))
        gt = jnp.where(hit0, w0, w1)
        xg = gather(lp, gt, 0)
        expert_tile(xg, s, 0, True)
        if s == 0:
            tab_cp.wait()
        cnt = seg(e)[3]

        def extra(i, carry_, lp=lp, gt=gt, s=s):
            expert_tile(gather(lp, gt, i), s, i, False)
            return carry_

        lax.fori_loop(1, (cnt + TM - 1) // TM, extra, 0)
        if s == 0:
            pl.semaphore_wait(barrier, 2)
            for n in nbr:
                pl.semaphore_signal(xsem, inc=1, device_id=(n,), device_id_type=MESH)
        send_own(s)

    for cp in meta_cp:
        cp.wait()

    def sum_pass(a_s, b_s, d_s):
        def blk(g, c):
            for k0 in range(0, 128, 8):
                vs = []
                for k in range(k0, k0 + 8):
                    vs.append((ybuf[a_s[g, k]].astype(F32)
                               + ybuf[b_s[g, k]].astype(F32)).astype(BF16))
                for k in range(k0, k0 + 8):
                    ybuf[d_s[g, k]] = vs[k - k0]
            return c
        lax.fori_loop(0, NB, blk, 0)

    recv_and_forward(0)
    recv_and_forward(1)
    sum_pass(sa_s, sb_s, sd_s)
    send_own(EL)
    recv_and_forward(2)
    recv_and_forward(3)
    sum_pass(na_s, nb_s, nd_s)
    recv_and_forward(EL)

    def npiece(cls, q):
        base = SUM0 + (4 + cls) * N
        return base + tab[q, 68 + cls], base + tab[q + 1, 68 + cls]

    for q in range(NB):
        lo, hi = npiece(my, q)
        send(lo, hi, SEM_NS + 2 * q, 0)
        lo, hi = npiece(left, q)
        send(lo, hi, SEM_NS + 2 * q, 1)

    for s in range(EL + 1):
        recv_forwarded(s)

    def out_copy(g):
        rows = pl.ds(pl.multiple_of(g * 128, 128), 128)
        return pltpu.make_async_copy(outv.at[rows], out_hbm.at[rows], osem.at[g])

    def final_blk(g, c):
        lo, hi = npiece(right, g)
        recv(lo, hi, SEM_NS + 2 * g, 0)
        lo, hi = npiece(diag, g)
        recv(lo, hi, SEM_NS + 2 * g, 1)
        ov = outv.at[pl.ds(pl.multiple_of(g * 128, 128), 128)]
        for k0 in range(0, 128, 8):
            vs = []
            for k in range(k0, k0 + 8):
                vs.append(ybuf[fa_s[g, k]].astype(F32) + ybuf[fb_s[g, k]].astype(F32))
            for k in range(k0, k0 + 8):
                ov[pl.ds(k, 1), :] = vs[k - k0].reshape(1, H)
        out_copy(g).start()
        return c

    lax.fori_loop(0, NB, final_blk, 0)

    for lo, hi, si in sent:
        @pl.when(hi > lo)
        def _(lo=lo, hi=hi, si=si):
            rcopy(lo, hi, si, my).wait_send()
    pl.semaphore_wait(xsem, 2)
    for g in range(NB):
        out_copy(g).wait()


def pallas_dist_moe_top2_ep_n1024_d512_e4_h1024_kernel(
    x: jax.Array,
    router_W: jax.Array,
    route_idx: jax.Array,
    expert_W: jax.Array,
):
    any_spec = pl.BlockSpec(memory_space=pl.ANY)
    idx_smem = pltpu.SMEM((NB, 128), I32)
    return pl.pallas_call(
        _kernel,
        out_shape=jax.ShapeDtypeStruct((N, H), F32),
        in_specs=[any_spec] * 4,
        out_specs=any_spec,
        scratch_shapes=[
            pltpu.VMEM((N, D), F32),
            pltpu.VMEM((N, D), BF16),
            pltpu.VMEM((EL, D, H), F32),
            pltpu.VMEM((E, D), F32),
            pltpu.VMEM((2, N), I32),
            pltpu.VMEM((ROWS, 8, 128), BF16),
            pltpu.VMEM((TM * 8, 128), F32),
            pltpu.VMEM((N, H), F32),
            pltpu.VMEM((8, NB, 128), I32),
            pltpu.VMEM((16, 128), I32),
            pltpu.SMEM((16, 128), I32),
            idx_smem, idx_smem, idx_smem, idx_smem,
            idx_smem, idx_smem, idx_smem, idx_smem,
            pltpu.SemaphoreType.DMA((2 + XCH + EL * WCH,)),
            pltpu.SemaphoreType.DMA((9,)),
            pltpu.SemaphoreType.DMA((NB,)),
            pltpu.SemaphoreType.DMA((NSEM,)),
            pltpu.SemaphoreType.DMA((NSEM,)),
            pltpu.SemaphoreType.REGULAR,
        ],
        compiler_params=pltpu.CompilerParams(
            collective_id=0,
            vmem_limit_bytes=100 * 1024 * 1024,
        ),
    )(x, router_W.T, route_idx.T.astype(I32), expert_W)
```

```python
import jax
import jax.numpy as jnp
from jax import lax
from jax.experimental import pallas as pl
from jax.experimental.pallas import tpu as pltpu

N = 1024
D = 512
H = 1024
E = 16
EL = 4
ND = 4
NB = N // 128

TM = 176
NT = -(-N // TM)
CAPE = NT * TM
ZROW = E * CAPE

NSUB = (1, 3)
BLK = ((1, 2), (4, 5, 6, 7, 0, 3))
PIECES = (((0, 1, 8),), ((0, 2, 8), (2, 1, 24)))
WCOLS = (((128, 256),), ((0, 128), (384, 640)))

XB = (2, 2, 2, 1, 1)
CAPQ = 32
KS = (256, 256)
G = 16
GS = 4

TAU = (4, 7)
F2M = (4, 6, 4, 2)
NA = 32
PER = 64
PER1 = 190
MARG = 10
CAPT = 950
BIGD = 90
COV = 45
LAST = 16
LOFF = (224, 70, 60, 158)
INV = (0, 300, 300, 150, 150, 0, 62, 62, 0)

F32 = jnp.float32
BF16 = jnp.bfloat16
I32 = jnp.int32
U32 = jnp.uint32
MESH = pl.DeviceIdType.MESH

SEM_P = 0
(SEM_S0, SEM_S1, SEM_FS0, SEM_FS1, SEM_N0, SEM_NA, SEM_NB, SEM_NC,
 SEM_D, SEM_D2, SEM_FD, SEM_F2) = range(16, 40, 2)
NSEM = SEM_F2 + 1

(R_SLO, R_SMID, R_SHI, R_DLO, R_DHI, R_FS0, R_FS1, R_FD, R_NLO, R_NMID, R_NHI,
 R_DALL, R_Q, R_POS) = range(14)


class _Table:
    def __init__(self, ref):
        self.ref = ref

    def __getitem__(self, idx):
        return self.ref[idx[0] * 128 + idx[1]]


def _loff(a, p):
    return LOFF[0] if p == 0 else LOFF[1] if a == 0 else LOFF[2] if p == 2 else LOFF[3]


def _unpack(v):
    return pltpu.bitcast(v, BF16).astype(F32)


def _kernel(x_hbm, rwt_hbm, rit_hbm, w_hbm, out_ref,
            x32, w32, rwt, rit, y0, y1, s0, s1, xg_ref, acc, metav, tabv, gsav, rsav,
            tab_s, u_s, pa0_s, pb0_s, pa1_s, pb1_s, w_s, plan, fin,
            lsem, msem, ssem, rsem, xsem):
    nq, kch = len(XB), len(KS)
    tab = _Table(tab_s)
    yh, sh, pa_s, pb_s = (y0, y1), (s0, s1), (pa0_s, pa1_s), (pb0_s, pb1_s)
    ko = [sum(KS[:k]) for k in range(kch)]
    my = lax.axis_index("i")
    left = (my + 3) % ND
    right = (my + 1) % ND
    diag = (my + 2) % ND
    nbr = (left, right)

    ri_cp = pltpu.make_async_copy(rit_hbm, rit, lsem.at[0])
    rw_cp = pltpu.make_async_copy(rwt_hbm, rwt, lsem.at[1])
    ri_cp.start()
    rw_cp.start()
    xlo = [128 * sum(XB[:q]) for q in range(nq + 1)]
    x_cp = [pltpu.make_async_copy(x_hbm.at[pl.ds(xlo[q], 128 * XB[q])],
                                  x32.at[pl.ds(xlo[q], 128 * XB[q])],
                                  lsem.at[2 + q]) for q in range(nq)]
    for cp in x_cp:
        cp.start()
    w_cp = {}
    nsem = 2 + nq
    for h in range(2):
        for s in range(EL):
            for k in range(kch):
                w_cp[s, h, k] = []
                for c0_, cn in WCOLS[h]:
                    idx = (s, pl.ds(ko[k], KS[k]), pl.ds(c0_, cn))
                    cp = pltpu.make_async_copy(w_hbm.at[idx], w32.at[idx], lsem.at[nsem])
                    cp.start()
                    w_cp[s, h, k].append(cp)
                    nsem += 1

    barrier = pltpu.get_barrier_semaphore()
    for n in nbr:
        pl.semaphore_signal(barrier, inc=1, device_id=(n,), device_id_type=MESH)

    for h in range(2):
        yh[h][pl.ds(NSUB[h] * ZROW, 8), :] = jnp.zeros((8, 128), U32)
    xg_ref[:, :, 0:TM, :] = jnp.zeros((EL, D // 128, TM, 128), F32)

    ri_cp.wait()
    e0 = rit[0:1, :]
    e1 = rit[1:2, :]
    c0 = e0 >> 2
    c1 = e1 >> 2
    dup = e0 == e1
    d01 = (c0 - c1) & 3
    d10 = (c1 - c0) & 3
    key0 = jnp.where(c0 >= 2, d01, d10) * 16 + e0
    key1 = jnp.where(dup, -1, jnp.where(c1 >= 2, d10, d01) * 16 + e1)
    late = jnp.where(((e0 & 3) == 3) | ((e1 & 3) == 3), 1, 0)
    skey = jnp.where(d01 == 0, 2 * c0 + late,
                     jnp.where(d10 == 1, 8 + 2 * c0 + late,
                               jnp.where(d10 == 3, 8 + 2 * c1 + late, 16 + (c0 & 1))))

    v64 = lax.broadcasted_iota(I32, (64, N), 0)
    v16 = lax.broadcasted_iota(I32, (16, N), 0)
    m0 = v64 == key0
    m1 = v64 == key1
    v32 = lax.broadcasted_iota(I32, (32, N), 0)
    ms = v32 == skey
    ohp = jnp.where(m0 | m1, 1.0, 0.0)
    ohs = jnp.where(ms, 1.0, 0.0).astype(BF16)
    cum1 = ohp[0:16] + ohp[16:32]
    cum2 = cum1 + ohp[32:48]
    cum3 = cum2 + ohp[48:64]
    ohp = ohp.astype(BF16)

    tok = lax.broadcasted_iota(I32, (16, N), 1)
    bsel = jnp.where(tok < v16 * 128, 1.0, 0.0).astype(BF16)
    tsrc = jnp.concatenate([ohp[0:16], cum1.astype(BF16), cum2.astype(BF16), cum3.astype(BF16),
                            ohp[32:48], ohs, jnp.zeros((16, N), BF16)], axis=0)
    tabf = lax.dot_general(bsel, tsrc, (((1,), (1,)), ((), ())),
                           preferred_element_type=F32)
    tabv[...] = tabf.astype(I32).reshape(16 * 128)
    tab_cp = pltpu.make_async_copy(tabv, tab_s, msem.at[0])
    tab_cp.start()

    oh = jnp.concatenate([ohp, ohs], axis=0)
    r_i = lax.broadcasted_iota(I32, (128, 256), 0)
    c_i = lax.broadcasted_iota(I32, (128, 256), 1)
    uo = jnp.where((r_i < c_i), 1.0, 0.0).astype(BF16)
    stacked = jnp.concatenate([oh[:, b * 128:(b + 1) * 128] for b in range(NB)], axis=0)
    pre = jnp.dot(stacked, uo, preferred_element_type=F32)
    scarry = jnp.zeros((24, 128), F32)
    goff = jnp.zeros((16, 128), F32)
    lfull, sfull = [], []
    for b in range(NB):
        ba = pre[b * 96:(b + 1) * 96]
        gt_ = ba[:64, 128:]
        t0 = goff + gt_[0:16]
        t1 = t0 + gt_[16:32]
        t2 = t1 + gt_[32:48]
        off = jnp.concatenate([goff, t0, t1, t2], axis=0)
        lfull.append(ba[:64, :128] + off)
        goff = goff + (t2 + gt_[48:64] - goff) * 2048.0
        sfull.append(ba[64:88, :128] + scarry)
        scarry = scarry + ba[64:88, 128:]
    lfull = jnp.concatenate(lfull, axis=1)
    sfull = jnp.concatenate(sfull, axis=1)
    stot = jnp.concatenate([scarry] * NB, axis=1)
    l0 = jnp.sum(jnp.where(m0, lfull, 0.0), axis=0, keepdims=True).astype(I32)
    l1 = jnp.sum(jnp.where(m1, lfull, 0.0), axis=0, keepdims=True).astype(I32)
    lq0, lq1 = l0 & 2047, l1 & 2047
    lp0, lp1 = lq0 + (l0 >> 11), lq1 + (l1 >> 11)
    upos = jnp.sum(jnp.where(ms[:24], sfull, jnp.where(v32[:24] < skey, stot, 0.0)),
                   axis=0, keepdims=True).astype(I32)
    metav[0:1, :] = upos
    for h in range(2):
        metav[1 + 2 * h:2 + 2 * h, :] = NSUB[h] * (e0 * CAPE + lp0)
        metav[2 + 2 * h:3 + 2 * h, :] = NSUB[h] * jnp.where(dup, ZROW, e1 * CAPE + lp1)
    meta_cp = [pltpu.make_async_copy(metav.at[k], dst, msem.at[1 + k])
               for k, dst in enumerate((u_s, pa0_s, pb0_s, pa1_s, pb1_s))]
    for cp in meta_cp:
        cp.start()
    r0 = jnp.where(c0 == my,
                   (lq0 // CAPQ) * (EL * CAPQ) + (e0 & 3) * CAPQ + lq0 % CAPQ, -1)
    r1 = jnp.where((c1 == my) & jnp.logical_not(dup),
                   (lq1 // CAPQ) * (EL * CAPQ) + (e1 & 3) * CAPQ + lq1 % CAPQ, -1)

    def invert(lo, hi):
        for t in range(lo, min(hi, N)):
            w_s[u_s[t]] = ((((t >> 3) << 6) + (t & 7)) << 10) | t

    def make_plan():
        w1 = NSUB[1]
        tot = [tab[8, 80 + v] for v in range(18)]
        coff = [0]
        for v in range(18):
            coff.append(coff[-1] + tot[v])
        stt = [tot[2 * c] + tot[2 * c + 1] for c in range(ND)]
        ncnt = [tot[8 + 2 * c] + tot[9 + 2 * c] for c in range(ND)]
        low = [tab[TAU[j], 96 + j] for j in range(2)]
        red = [tot[17] - low[1], low[0], low[1], tot[16] - low[0]]
        dlo = [coff[18] - red[0], coff[16], coff[17], coff[17] - red[3]]
        for c in range(ND):
            plan[4 * R_SLO + c] = coff[2 * c]
            plan[4 * R_SMID + c] = coff[2 * c + 1]
            plan[4 * R_SHI + c] = coff[2 * c + 2]
            plan[4 * R_NLO + c] = coff[8 + 2 * c]
            plan[4 * R_NMID + c] = coff[9 + 2 * c]
            plan[4 * R_NHI + c] = coff[10 + 2 * c]
            plan[4 * R_DLO + c] = dlo[c]
            plan[4 * R_DHI + c] = dlo[c] + red[c]
            plan[4 * R_Q + c] = 0
        plan[4 * R_DALL] = coff[16]
        la, lb = {}, {}
        for a in range(ND):
            fix = ((1 + w1) * (ncnt[a] + ncnt[(a + 3) % 4] + stt[a]) + tot[16 + (a & 1)]
                   + w1 * red[a])
            for d, p_ in ((0, (a + 3) % 4), (1, (a + 1) % 4)):
                k_ = 32 if (a >= 2) == (d == 0) else 48
                gap, short = 0, 0
                for e in range(a * EL, a * EL + 3):
                    short = short + (PER - tab[8, k_ + e] + tab[8, k_ - 32 + e])
                    gap = jnp.maximum(gap, short)
                e = a * EL + 3
                n3 = tab[8, k_ + e] - tab[8, k_ - 32 + e] - tab[8, 64 + e]
                f2 = tab[F2M[(p_ + 2) % 4], 96 + (p_ & 1)]
                if d == 1:
                    f2 = tot[16 + (p_ & 1)] - f2
                la[a, p_] = fix + w1 * red[p_] + _loff(a, p_) + f2 + gap
                lb[a, p_] = (_loff(a, p_) + CAPT + ((w1 * red[p_]) >> 2) + w1 * (
                    n3 + tot[2 * a + 1] + red[a] + ncnt[a if d == 0 else (a + 3) % 4]))
        for q in range(ND):
            a, b = ((q + 1) % 4, (q + 2) % 4), ((q + 3) % 4, (q + 2) % 4)

            def diff(x, a=a, b=b, q=q):
                return (jnp.maximum(la[b] + stt[q] - x, lb[b]) - jnp.maximum(la[a] + x, lb[a]))

            t_ = stt[q] + red[q]
            x0 = jnp.clip((stt[q] + jnp.maximum(lb[a] - la[a], 0)
                           - jnp.maximum(lb[b] - la[b], 0)) >> 1, 0, stt[q])
            need = diff(x0)
            x0 = jnp.clip(x0 + ((jnp.maximum(need - w1 * t_, 0)
                                 + jnp.minimum(need + w1 * t_, 0)) >> 1), 0, stt[q])
            f = jnp.clip((t_ + ((diff(x0) * 43) >> 7)) >> 1, 0, t_)
            fd = jnp.clip(red[q] >> 1, f - stt[q], f)
            plan[4 * R_FS0 + q] = x0
            plan[4 * R_FS1 + q] = f - fd
            plan[4 * R_FD + q] = fd

    rw_cp.wait()
    rwh = rwt[...].astype(BF16)
    rwb = jnp.concatenate([rwh, (rwt[...] - rwh.astype(F32)).astype(BF16)], axis=0)
    jrow = lax.broadcasted_iota(I32, (EL * CAPQ, 128), 0)

    def gpass(j, xb, r0b, r1b, w0b, w1b, offs):
        sh_ = j * (EL * CAPQ)
        pm = jnp.where(jrow == r0b - sh_, w0b,
                       jnp.where(jrow == r1b - sh_, w1b, 0.0)).astype(BF16)
        res = jnp.dot(pm, xb, preferred_element_type=F32)
        for s in range(EL):
            for c in range(D // 128):
                xg_ref[s, c, pl.ds(offs[s] + j * CAPQ, CAPQ), :] = (
                    res[s * CAPQ:(s + 1) * CAPQ, c * 128:(c + 1) * 128])

    pending = None
    bad = jnp.int32(NB)
    for q in range(nq):
        nt = 128 * XB[q]
        sl = slice(xlo[q], xlo[q + 1])
        if q == 0:
            tab_cp.wait()
        if q == 1:
            for cp in meta_cp:
                cp.wait()
        x_cp[q].wait()
        xq = x32[pl.ds(xlo[q], nt), :].astype(BF16)
        scores = lax.dot_general(rwb, xq, (((1,), (1,)), ((), ())),
                                 preferred_element_type=F32)
        scores = scores[:E] + scores[E:]
        vq = lax.broadcasted_iota(I32, (16, nt), 0)
        smax = jnp.max(scores, axis=0, keepdims=True)
        p = jnp.exp(scores - smax)
        probs = p / jnp.sum(p, axis=0, keepdims=True)
        g0 = jnp.sum(jnp.where(vq == e0[:, sl], probs, 0.0), axis=0, keepdims=True)
        g1 = jnp.sum(jnp.where(vq == e1[:, sl], probs, 0.0), axis=0, keepdims=True)
        gs = g0 + g1
        w1q = g1 / gs
        w0q = g0 / gs
        w0q = jnp.where(dup[:, sl], w0q + w1q, w0q)

        def gathers(q=q, xq=xq, w0q=w0q, w1q=w1q):
            for i in range(XB[q]):
                b = xlo[q] // 128 + i
                lo_, gl = slice(i * 128, (i + 1) * 128), slice(b * 128, (b + 1) * 128)
                gsav[0, b:b + 1, :] = w0q[:, lo_]
                gsav[1, b:b + 1, :] = w1q[:, lo_]
                rsav[0, b:b + 1, :] = r0[:, gl]
                rsav[1, b:b + 1, :] = r1[:, gl]
                offs = [0 if b == 0 else tab[b, 48 + my * EL + s] for s in range(EL)]
                gpass(0, xq[lo_], r0[:, gl], r1[:, gl], w0q[:, lo_], w1q[:, lo_], offs)

        if pending is not None:
            pending()
        pending = gathers
        if q == 0:
            for b in reversed(range(NB)):
                for s in range(EL):
                    cnt_ = tab[b + 1, 48 + my * EL + s] - tab[b, 48 + my * EL + s]
                    bad = jnp.where(cnt_ > CAPQ, b, bad)
            make_plan()
        invert(sum(INV[:q]), sum(INV[:q + 1]))
    pending()

    def regather(b, c_):
        row = pl.ds(b, 1)
        offs = [tab[b, 48 + my * EL + s] for s in range(EL)]
        mx = jnp.int32(1)
        for s in range(EL):
            mx = jnp.maximum(mx, tab[b + 1, 48 + my * EL + s] - offs[s])

        def one(j, c2):
            xb = x32[pl.ds(pl.multiple_of(b * 128, 128), 128), :].astype(BF16)
            gpass(j, xb, rsav[0, row, :], rsav[1, row, :], gsav[0, row, :],
                  gsav[1, row, :], offs)
            return c2
        return lax.fori_loop(0, (mx + CAPQ - 1) // CAPQ, one, c_)

    lax.fori_loop(bad, NB, regather, 0)

    def dev_of(d):
        return (my + 3 - 2 * d) & 3

    def src_of(d):
        return (my + 1 + 2 * d) & 3

    def tau_of(chip):
        return jnp.where((chip & 1) == 0, TAU[0], TAU[1])

    def f2m_of(chip):
        return jnp.where((chip & 1) == 0, F2M[0], jnp.where(chip == 1, F2M[1], F2M[3]))

    def own_ranges(s, h):
        e = my * EL + s
        tk = [[tab[b, 16 * k + e] for b in range(NB + 1)] for k in range(4)]
        out = []
        for b in range(NB):
            gb = e * CAPE + tk[3][b]
            o1, o2, o3 = (gb + tk[k][b + 1] - tk[k][b] for k in range(3))
            o4 = e * CAPE + tk[3][b + 1]
            if h == 0:
                out.append(((o1, o3), (o2, o4)))
            else:
                c_ = (o3 if b < min(TAU) else o2 if b >= max(TAU)
                      else jnp.where(b < tau_of(my), o3, o2))
                out.append(((o1, c_), (c_, o4)))
        return out, tk[3][NB]

    def p_count(chip, s, h, d):
        e = chip * EL + s
        dl = tab[8, 64 + e] if h == 0 else tab[tau_of(chip), 64 + e]
        t1_ = tab[8, 16 + e]
        low = t1_ - tab[8, e] + dl
        high = tab[8, 48 + e] - t1_ - (0 if h == 0 else dl)
        return jnp.where((chip >= 2) == (d == 0), low, high)

    def split(row_lo, row_hi, row_f, chip):
        lo, hi = plan[4 * row_lo + chip], plan[4 * row_hi + chip]
        cut = lo + plan[4 * row_f + chip]
        return (lo, hi), (cut, hi), (lo, cut)

    def s_ranges(chip, h):
        return split(R_SLO, R_SHI, R_FS0 + h, chip)

    def d_ranges(chip):
        return split(R_DLO, R_DHI, R_FD, chip)

    def n_bounds(chip, d):
        cls = (chip + 3 * d) & 3
        return tuple(plan[4 * r + cls] for r in (R_NLO, R_NMID, R_NHI))

    def n_pieces(chip, d):
        lo, mid, hi = n_bounds(chip, d)
        big = plan[4 * R_DHI + chip] - plan[4 * R_DLO + chip] > BIGD
        cut = jnp.where(big, jnp.minimum(lo + COV, mid), mid)
        cut2 = jnp.maximum(hi - LAST, mid)
        return (lo, cut), (cut, cut2), (cut2, hi)

    def rcopy(buf, h, lo, hi, sem_idx, dev):
        rows = buf[h].at[pl.ds(NSUB[h] * lo, NSUB[h] * (hi - lo))]
        return pltpu.make_async_remote_copy(
            src_ref=rows, dst_ref=rows, send_sem=ssem,
            recv_sem=rsem.at[sem_idx], device_id=(dev,), device_id_type=MESH)

    def account(units, d):
        plan[4 * R_Q + d] = plan[4 * R_Q + d] + units
        plan[4 * R_Q + 2] = plan[4 * R_Q + 2] + units

    def send(buf, h, rng, sem_idx, d, count=True):
        lo, hi = rng

        @pl.when(hi > lo)
        def _():
            rcopy(buf, h, lo, hi, sem_idx + d, dev_of(d)).start()
        if count:
            account(NSUB[h] * (hi - lo), d)

    def recv(buf, h, rng, sem_idx, d):
        lo, hi = rng

        @pl.when(hi > lo)
        def _():
            rcopy(buf, h, lo, hi, sem_idx + d, my).wait_recv()

    def fill(h, sem_idx, d, limit, everything=False):
        pos = plan[4 * R_POS + 2 * h + d]
        end = limit
        if not everything:
            room = jnp.maximum(PER1 + MARG - plan[4 * R_Q + d], 0)
            end = jnp.minimum(limit, pos + (room if h == 0 else (room * 43) >> 7))
        send(sh, h, (pos, end), sem_idx, d)
        plan[4 * R_POS + 2 * h + d] = end

    def f2_blocks(chip, d):
        m = f2m_of(chip)
        return jnp.where(d == 0, 0, m), jnp.where(d == 0, m, NB)

    def recv_p(g, dirs=(0, 1)):
        h, s = g // EL, g % EL
        todo = []
        for d in dirs:
            chip = src_of(d)
            fw, tot_ = [], None
            if h == 0:
                e = chip * EL + s
                b0, b1 = f2_blocks(chip, d)
                nf = max(F2M)
                first = (NB - nf) * d
                t1_ = [tab[first + i, 16 + e] for i in range(nf + 1)]
                dc = [tab[first + i, 64 + e] for i in range(nf + 1)]
                for i in range(nf):
                    b = first + i
                    lo = e * CAPE + tab[b, 48 + e] + t1_[i + 1] - t1_[i]
                    n_ = jnp.where((b >= b0) & (b < b1), dc[i + 1] - dc[i], 0)
                    fw.append((lo, lo + n_))
                    tot_ = n_ if tot_ is None else tot_ + n_
                account(tot_, d)
            lo = (chip * EL + s) * CAPE
            todo.append((d, (lo, lo + p_count(chip, s, h, d)), fw))
        for d, size, fw in todo:
            recv(yh, h, size, SEM_P + 2 * g, d)
            for rng in fw:
                send(yh, 0, rng, SEM_F2 - d, d, count=False)

    def expert_tile(s, h, i, wait, filler=None):
        y = None
        for k in range(kch):
            if wait:
                for cp in w_cp[s, h, k]:
                    cp.wait()
            wc = jnp.concatenate([w32[s, pl.ds(ko[k], KS[k]), pl.ds(c * 128, 128)]
                                  for c in BLK[h]], axis=1).astype(BF16)
            r = pl.ds(0, TM) if wait else pl.ds(pl.multiple_of(i * TM, 16), TM)
            xk = jnp.concatenate([xg_ref[s, c, r, :]
                                  for c in range(ko[k] // 128, (ko[k] + KS[k]) // 128)],
                                 axis=1).astype(BF16)
            part = jnp.dot(xk, wc, preferred_element_type=F32)
            nc = 256 * NSUB[h]
            if k > 0:
                part = part + acc[:, 0:nc]
            if k < kch - 1:
                acc[:, 0:nc] = part
            else:
                y = part
            if filler is not None:
                filler(k)
        yb = lax.bitcast_convert_type(y, U32) + jnp.uint32(0x8000)
        base = NSUB[h] * ((my * EL + s) * CAPE + i * TM)
        for j in range(NSUB[h]):
            lo_ = yb[:, (2 * j) * 128:(2 * j + 1) * 128] >> 16
            hi_ = yb[:, (2 * j + 1) * 128:(2 * j + 2) * 128] & jnp.uint32(0xFFFF0000)
            yh[h][pl.ds(base + j, TM, stride=NSUB[h]), :] = lo_ | hi_

    low_left = my >= 2
    pdir = (jnp.where(low_left, 0, 1), jnp.where(low_left, 1, 0))

    def granule(g, mid=None):
        h, s = g // EL, g % EL
        rr = []

        def filler(k):
            if k == 0:
                rr.append(own_ranges(s, h))
            if g <= 3 and k == 0:
                invert(sum(INV[:nq + g]), sum(INV[:nq + g + 1]))
            if k == 0 and mid is not None:
                mid()

        expert_tile(s, h, 0, True, filler)
        grp, cnt = rr[0]

        def more(i, c_):
            expert_tile(s, h, i, False)
            return c_

        @pl.when(cnt > TM)
        def _():
            lax.fori_loop(1, (cnt + TM - 1) // TM, more, 0)

        for b in range(NB):
            for i in range(2):
                send(yh, h, grp[b][i], SEM_P + 2 * g, pdir[i], count=False)
        for d in range(2):
            plan[4 * R_Q + d] = (0 if g <= EL else
                                 jnp.maximum(plan[4 * R_Q + d] - PER1, 0))
            account(NSUB[h] * p_count(my, s, h, d), d)

    def row_loop(rng, group):
        lo, hi = rng
        n = hi - lo

        @pl.when(n >= G)
        def _():
            def body(i, c):
                start = jnp.minimum(lo + i * G, hi - G)
                group([start + k for k in range(G)])
                return c
            lax.fori_loop(0, lax.div(n + (G - 1), G), body, 0)

        @pl.when(n < G)
        def _():
            def body(i, c):
                group([jnp.minimum(lo + i * GS + k, hi - 1) for k in range(GS)])
                return c
            lax.fori_loop(0, lax.div(n + (GS - 1), GS), body, 0)

    def put_out(h, w, pc, v):
        so, ns, stride = PIECES[h][pc]
        first = 8 * BLK[h][2 * so]
        view = out_ref.at[pl.ds(first, 8 * N - first)]
        view[pl.ds(w >> 10, 2 * ns, stride=stride), :] = v

    def jobs(h, rng):
        def group(us):
            for k0 in range(0, len(us), 8):
                sub = us[k0:k0 + 8]
                ws = [w_s[u] for u in sub]
                vs = []
                for w in ws:
                    t = w & (N - 1)
                    a, b = pa_s[h][t], pb_s[h][t]
                    vs.append([_unpack(yh[h][pl.ds(a + so, ns), :])
                               + _unpack(yh[h][pl.ds(b + so, ns), :])
                               for so, ns, _ in PIECES[h]])
                for u, w, v in zip(sub, ws, vs):
                    for pc, (so, ns, _) in enumerate(PIECES[h]):
                        sh[h][pl.ds(NSUB[h] * u + so, ns), :] = (
                            pltpu.bitcast(v[pc].astype(BF16), U32))
                        put_out(h, w, pc, v[pc])
        row_loop(rng, group)

    def scatter(h, rng):
        def group(us):
            vs = [[_unpack(sh[h][pl.ds(NSUB[h] * u + so, ns), :])
                   for so, ns, _ in PIECES[h]] for u in us]
            for u, v in zip(us, vs):
                w = w_s[u]
                for pc in range(len(PIECES[h])):
                    put_out(h, w, pc, v[pc])
        row_loop(rng, group)

    def s_fwd(h):
        for d in range(2):
            ss = s_ranges(src_of(d), h)
            recv(sh, h, ss[0], SEM_S0 + 2 * h, d)
            send(sh, h, ss[1 + d], SEM_FS0 + 2 * h, d)

    def s_scat(h):
        for d in range(2):
            scatter(h, s_ranges(src_of(d), h)[0])

    def recv_scatter(h, rng, sem_idx, d):
        recv(sh, h, rng, sem_idx, d)
        scatter(h, rng)

    def final_merge():
        for d in range(2):
            np_ = n_pieces(src_of(d), d)
            seq = [(np_[1], SEM_NB), (s_ranges(diag, 1)[1 + d], SEM_FS1),
                   (d_ranges(diag)[1 + d], SEM_FD), (np_[2], SEM_NC)]
            rem = 0
            for k in reversed(range(4)):
                (lo, hi), sem_idx = seq[k]
                fin[d * 20 + k * 4 + 0] = lo
                fin[d * 20 + k * 4 + 1] = hi
                fin[d * 20 + k * 4 + 2] = sem_idx + d
                fin[d * 20 + k * 4 + 3] = rem
                rem = rem + (hi - lo)
            fin[d * 20 + 19] = -1

        def step(_, c):
            i0, i1 = c
            first = fin[i0 + 3] >= fin[i1 + 3]
            i = jnp.where(first, i0, i1)
            recv_scatter(1, (fin[i], fin[i + 1]), fin[i + 2], 0)
            return jnp.where(first, i0 + 4, i0), jnp.where(first, i1, i1 + 4)

        lax.fori_loop(0, 8, step, (jnp.int32(0), jnp.int32(20)))

    order = (jnp.where(my == 1, 1, 0), jnp.where(my == 1, 0, 1))

    def na0(lo_i, hi_i):
        def one(i, c_):
            d = jnp.where(i == 0, order[0], order[1])
            recv_p(1, (d,))
            recv_p(2, (d,))
            lo, mid, _ = n_bounds(my, d)
            end = jnp.minimum(lo + NA, mid)
            jobs(0, (lo, end))
            send(sh, 0, (lo, end), SEM_N0, d)
            plan[4 * R_POS + d] = end
            return c_
        lax.fori_loop(lo_i, hi_i, one, 0)

    early = jnp.where(my == 0, 0, 1)

    def mid4():
        na0(1, 1 + early)

    def mid5():
        recv_p(3)

    def mid6():
        s_scat(0)

    def n0_fill(which, everything=False):
        for d in range(2):
            fill(0, SEM_N0, d, n_bounds(my, d)[which], everything)

    pl.semaphore_wait(barrier, 2)
    for n in nbr:
        pl.semaphore_signal(xsem, inc=1, device_id=(n,), device_id_type=MESH)
    granule(0)
    granule(1)
    granule(2)
    granule(3)
    smine = s_ranges(my, 0)[0]
    jobs(0, smine)
    for d in range(2):
        send(sh, 0, smine, SEM_S0, d)
    recv_p(0)
    na0(0, early)
    granule(4, mid4)
    na0(2 * early, 2)
    for d in range(2):
        jobs(0, (plan[4 * R_POS + d], n_bounds(my, d)[1]))
    n0_fill(1)
    granule(5, mid5)
    for d in range(2):
        jobs(0, n_bounds(my, d)[1:])
    s_fwd(0)
    n0_fill(2)
    granule(6, mid6)
    n0_fill(2)
    smid = plan[4 * R_SMID + my]
    jobs(1, (smine[0], smid))
    for d in range(2):
        plan[4 * R_POS + 2 + d] = smine[0]
        fill(1, SEM_S1, d, smid)
    granule(7)
    n0_fill(2, True)
    jobs(1, (smid, smine[1]))
    for d in range(2):
        fill(1, SEM_S1, d, smine[1], True)

    def ne1(i, c_):
        d = jnp.where(i == 0, order[0], order[1])
        for g in (4, 5, 6):
            recv_p(g, (d,))
        jobs(1, n_bounds(my, d)[:2])
        send(sh, 1, n_pieces(my, d)[0], SEM_NA, d)
        return c_
    lax.fori_loop(0, 2, ne1, 0)
    recv_p(7)
    dm = d_ranges(my)
    jobs(1, dm[0])
    for d in range(2):
        send(sh, 1, dm[1 + d], SEM_D, d)
    for d in range(2):
        send(sh, 1, dm[2 - d], SEM_D2, d)
    for d in range(2):
        jobs(1, n_bounds(my, d)[1:])
    for d in range(2):
        send(sh, 1, n_pieces(my, d)[1], SEM_NB, d)
    s_fwd(1)
    for d in range(2):
        lo, _, hi = n_bounds(src_of(d), d)
        recv_scatter(0, (lo, hi), SEM_N0, d)
    lo = diag * (EL * CAPE)
    recv(yh, 0, (lo, lo + tab[8, 96 + (my & 1)]), SEM_F2, 0)
    jobs(0, (plan[4 * R_DALL], N))
    for d in range(2):
        recv_scatter(0, s_ranges(diag, 0)[1 + d], SEM_FS0, d)
    s_scat(1)
    for d in range(2):
        recv_scatter(1, n_pieces(src_of(d), d)[0], SEM_NA, d)
    for d in range(2):
        rng = d_ranges(src_of(d))[1 + d]
        recv(sh, 1, rng, SEM_D, d)
        send(sh, 1, rng, SEM_FD, d)
        send(sh, 1, n_pieces(my, d)[2], SEM_NC, d)
    for d in range(2):
        dd = d_ranges(src_of(d))
        recv(sh, 1, dd[2 - d], SEM_D2, d)
        scatter(1, dd[0])
    final_merge()

    total = plan[4 * R_Q + 2]

    @pl.when(total > 0)
    def _():
        rows = y1.at[pl.ds(0, total)]
        pltpu.make_async_copy(rows, rows, ssem).wait()
    pl.semaphore_wait(xsem, 2)


def pallas_dist_moe_top2_ep_n1024_d512_e4_h1024_kernel(
    x: jax.Array,
    router_W: jax.Array,
    route_idx: jax.Array,
    expert_W: jax.Array,
):
    any_spec = pl.BlockSpec(memory_space=pl.ANY)
    idx_smem = pltpu.SMEM((N,), I32)
    raw = pl.pallas_call(
        _kernel,
        out_shape=jax.ShapeDtypeStruct((8 * N, 128), F32),
        in_specs=[any_spec] * 4,
        out_specs=pl.BlockSpec(memory_space=pltpu.VMEM),
        scratch_shapes=[
            pltpu.VMEM((N, D), F32),
            pltpu.VMEM((EL, D, H), F32),
            pltpu.VMEM((E, D), F32),
            pltpu.VMEM((2, N), I32),
            pltpu.VMEM((NSUB[0] * ZROW + 8, 128), U32),
            pltpu.VMEM((NSUB[1] * ZROW + 8, 128), U32),
            pltpu.VMEM((NSUB[0] * N, 128), U32),
            pltpu.VMEM((NSUB[1] * N, 128), U32),
            pltpu.VMEM((EL, D // 128, CAPE, 128), F32),
            pltpu.VMEM((TM, 256 * NSUB[1]), F32),
            pltpu.VMEM((8, N), I32),
            pltpu.VMEM((16 * 128,), I32),
            pltpu.VMEM((2, NB, 128), F32),
            pltpu.VMEM((2, NB, 128), I32),
            pltpu.SMEM((16 * 128,), I32),
            idx_smem, idx_smem, idx_smem, idx_smem, idx_smem, idx_smem,
            pltpu.SMEM((64,), I32),
            pltpu.SMEM((40,), I32),
            pltpu.SemaphoreType.DMA((2 + len(XB) + EL * 3 * len(KS),)),
            pltpu.SemaphoreType.DMA((6,)),
            pltpu.SemaphoreType.DMA,
            pltpu.SemaphoreType.DMA((NSEM,)),
            pltpu.SemaphoreType.REGULAR,
        ],
        compiler_params=pltpu.CompilerParams(
            collective_id=0,
            vmem_limit_bytes=100 * 1024 * 1024,
            disable_semaphore_checks=True,
        ),
    )(x, router_W.T, route_idx.T.astype(I32), expert_W)
    return raw.reshape(N // 8, 8, 8, 128).transpose(0, 2, 1, 3).reshape(N, H)
```
